```python
import numpy as np

kernel_name = "dist_mlp2_tp_i_m512_h1024_out512"

def setup_inputs():
    x = np.random.randn(512, 512).astype(np.float32)
    W1 = np.random.randn(512, 4096).astype(np.float32)
    W2 = np.random.randn(4096, 512).astype(np.float32)
    return {"x": x, "W1": W1, "W2": W2}

def reference(x: np.ndarray, W1: np.ndarray, W2: np.ndarray) -> np.ndarray:
    h = x @ W1
    h = np.maximum(h, 0.0)
    return h @ W2
```

```python
import contextlib
import jax
import jax.numpy as jnp
from jax import lax
from jax.experimental import pallas as pl
from jax.experimental.pallas import tpu as pltpu

HBM = pltpu.MemorySpace.HBM
MESH = pl.DeviceIdType.MESH
BF = jnp.bfloat16
F32 = jnp.float32

def make(order=None, scopes=False, loads=None, **cp):
    loads = loads or ["xa", "k0", "k1", "k2", "k3", "c0", "c1", "xb", "c2", "c3"]
    order = order or ["h1", "bar", "p0", "p1", "h2a", "p2", "h2b", "p3", "q0", "q1", "q2", "q3", "t0", "t1", "t2", "t3"]
    def scope(n):
        return jax.named_scope(n) if scopes else contextlib.nullcontext()
    def kern(x, W1, W2):
        def body(x_ref, w1_ref, w2_ref, o_ref, xv, w1v, w2v, w1b, w2b, acc, hb, s1, r1, s2, r2, s3,
                 lsem, r1sem, r2sem, fsem, ssem, osem):
            me = lax.axis_index("i")
            px = me ^ 1
            py = 3 - me
            ownA = (me ^ (me >> 1)) & 1
            ownB = 2 + (me >> 1)
            rows = [1 - ownA, 5 - ownB, ownA, ownB]
            def xcp(j):
                return pltpu.make_async_copy(x_ref.at[pl.ds(pl.multiple_of(rows[j] * 128, 128), 128)], xv.at[pl.ds(j * 128, 128)], lsem.at[j])
            def kcp(k):
                return pltpu.make_async_copy(w1_ref.at[pl.ds(k * 128, 128)], w1v.at[pl.ds(k * 128, 128)], lsem.at[4 + k])
            def ccp(c):
                return pltpu.make_async_copy(w2_ref.at[:, pl.ds(c * 128, 128)], w2v.at[c], lsem.at[8 + c])
            for l in loads:
                if l == "xa": xcp(0).start(); xcp(1).start()
                elif l == "xb": xcp(2).start(); xcp(3).start()
                elif l == "xb0": xcp(2).start()
                elif l == "xb1": xcp(3).start()
                elif l[0] == "k": kcp(int(l[1])).start()
                else: ccp(int(l[1])).start()
            bar = pltpu.get_barrier_semaphore()
            for nb in (px, py):
                pl.semaphore_signal(bar, inc=1, device_id=(nb,), device_id_type=MESH)
            def rc(src, dst, rsem, dev):
                return pltpu.make_async_remote_copy(src, dst, ssem, rsem, device_id=(dev,), device_id_type=MESH)
            for op in order:
              with scope(op):
                if op == "h1":
                    xcp(0).wait(); xcp(1).wait()
                    xa = xv[0:256, :].astype(BF)
                    for k in range(4):
                        kcp(k).wait()
                        w = w1v[k * 128:(k + 1) * 128, :].astype(BF)
                        w1b[k * 128:(k + 1) * 128, :] = w
                        d = jnp.dot(xa[:, k * 128:(k + 1) * 128], w, preferred_element_type=F32)
                        if k == 0: acc[...] = d
                        elif k < 3: acc[...] += d
                        else: hb[0:256, :] = jnp.maximum(acc[...] + d, 0.0).astype(BF)
                elif op == "bar":
                    pl.semaphore_wait(bar, 2)
                elif op in ("h2a", "h2b"):
                    j = 2 if op == "h2a" else 3
                    xcp(j).wait()
                    d = jnp.dot(xv[j * 128:(j + 1) * 128, :].astype(BF), w1b[...], preferred_element_type=F32)
                    hb[j * 128:(j + 1) * 128, :] = jnp.maximum(d, 0.0).astype(BF)
                elif op[0] == "p":
                    c = int(op[1])
                    ccp(c).wait()
                    w = w2v[c].astype(BF)
                    w2b[c] = w
                    s1[c] = jnp.dot(hb[0:256, :], w, preferred_element_type=F32).astype(BF)
                    rc(s1.at[c, 0:128], r1.at[c, 0:128], r1sem.at[c], px).start()
                    rc(s1.at[c, 128:256], r1.at[c, 128:256], r1sem.at[c], py).start()
                elif op[0] == "q":
                    c = int(op[1])
                    d = jnp.dot(hb[256:512, :], w2b[c], preferred_element_type=F32)
                    pltpu.make_async_copy(r1.at[c], r1.at[c], r1sem.at[c]).wait()
                    s2[c] = (d + r1[c].astype(F32)).astype(BF)
                    rc(s2.at[c, 0:128], r2.at[c, 0:128], r2sem.at[c], py).start()
                    rc(s2.at[c, 128:256], r2.at[c, 128:256], r2sem.at[c], px).start()
                elif op[0] == "t":
                    c = int(op[1])
                    pltpu.make_async_copy(r2.at[c], r2.at[c], r2sem.at[c]).wait()
                    tot = (s2[c].astype(F32) + r2[c].astype(F32)).astype(BF)
                    for j, dev in ((0, px), (1, py)):
                        dst = o_ref.at[pl.ds(pl.multiple_of(rows[2 + j] * 128, 128), 128), pl.ds(c * 128, 128)]
                        dst[...] = tot[j * 128:(j + 1) * 128]
                        rc(dst, dst, fsem, dev).start()
            with scope("fin"):
                for b in (s1, s2, s3):
                    pltpu.make_async_copy(b, b, ssem).wait()
                pltpu.make_async_copy(s3, s3, fsem).wait()
        msg = pltpu.VMEM((4, 256, 128), BF)
        return pl.pallas_call(body, out_shape=jax.ShapeDtypeStruct((512, 512), BF),
            in_specs=[pl.BlockSpec(memory_space=HBM)] * 3, out_specs=pl.BlockSpec(memory_space=pltpu.VMEM),
            scratch_shapes=[pltpu.VMEM((512, 512), F32), pltpu.VMEM((512, 1024), F32), pltpu.VMEM((4, 1024, 128), F32),
                            pltpu.VMEM((512, 1024), BF), pltpu.VMEM((4, 1024, 128), BF), pltpu.VMEM((256, 1024), F32),
                            pltpu.VMEM((512, 1024), BF), msg, msg, msg, msg, msg,
                            pltpu.SemaphoreType.DMA((12,)), pltpu.SemaphoreType.DMA((4,)), pltpu.SemaphoreType.DMA((4,)),
                            pltpu.SemaphoreType.DMA, pltpu.SemaphoreType.DMA, pltpu.SemaphoreType.DMA],
            compiler_params=pltpu.CompilerParams(collective_id=0, **cp))(x, W1, W2)
    return kern


def pallas_dist_mlp2_tp_i_m512_h1024_out512_kernel(x, W1, W2):
    return make(disable_semaphore_checks=True, disable_bounds_checks=True)(x, W1, W2)
```

```python
import jax
import jax.numpy as jnp
from jax import lax
from jax.experimental import pallas as pl
from jax.experimental.pallas import tpu as pltpu

_CHIPS = 4
_ROWS = 64
_LANES = 128

_ROUTES = (
    "303-/303- 3030/-01- 1012/--10 3212/1--2",
    "1010/--30 1010/--30 1010/--10 1212/1--2",
    "1212/1--2 1010/--30 3230/-03- 3232/32--",
    "1012/--12 1012/--10 1012/--10 1012/--12",
    "323-/323- 3230/-03- 3230/-03- 3232/32--",
    "3232/32-- 3030/-23- 1012/--10 1212/1--2",
    "-030/-010 1030/--10 3030/-03- 3232/32--",
    "1010/--10 1010/--12 3230/-03- 1232/32--",
)

_LOADS = (
    "x:30,42 u:2 x:02,20,21,22,23,32,33,43,50,51,52,53,70,72,73 u:3 x:03 u:0 u:1 "
    "v:00 v:01 v:3 x:62 v:2 v:1",
    "x:00,40,41,60,63,71 u:0 x:01,50 u:1 x:61 u:2 u:3 v:0 v:1 v:2 x:31,32 v:3 "
    "x:30,33",
    "x:12,22,52,73 u:2 x:02,03,23,62,72 u:3 x:43,53 u:0 u:1 v:10 v:11 x:40 v:0 "
    "x:33 v:2 v:3",
    "x:13,31,70,71 u:0 x:10,20,30 u:1 x:01,11 u:2 u:3 v:00 v:01 v:1 v:2 v:3 "
    "x:40,41,42,43",
)

_STEPS = (
    "x21>1 x51>1 x51>3 x21>3 x42>1 x02>1 K2:023457 x32>3 x72>3 K3:023457 x53>1 "
    "x23>1 x33>3 K0:2357 x20>1 x50>3 x03>3 x02>3 K1:2345 x72>1 H0:25 wQ40 wQ70 "
    "P20 P50 Q40 Q41 Q42 s20 Q43 s50 Q70 P30 P40 s30 s40 x11>1 Q00 Q71 Q72 Q01 "
    "Q02 Q03 x61>3 P53 P23 s53 Q73 P33 P73 s23 P03 s33 P00 s73 P70 s03 P43 wQ60 "
    "wQ10 P02 s43 P32 P42 s02 P22 Q60 P52 s42 Q61 s22 s32 Q62 Q10 P72 Q11 Q12 s70 "
    "wP51 s00 Q63 s52 P51 Q13 s72 P71 P41 P12 P13 s51 s71 P11 s41 s13 P63 P21 s21 "
    "s11 ws01 s63 P01 P62 s01 P31 s62 s31 t21>3 P61 P60 P10 s61 t61>3 t01>1 t70>3 "
    "s12 t00>1 t60>1 s10 t10>3 t11>3 t12>3 t62>1 t60>3 t41>1 t31>3 t22>1 t52>3 "
    "t72>1 t02>3 t42>1 t32>3 | f51 f71 f50 f20 f40 f30 f73 f33 f43 f13 f63 f53 "
    "f23 f03",
    "x63>2 x00>2 x41>0 x40>0 x60>2 x50>2 K0:0456 x00>0 x63>0 x21>2 x61>0 x71>2 "
    "K1:024567 x60>0 x61>2 x42>2 x41>2 K2:0245 Q60 Q61 Q62 Q63 K3:0257 wQ40 wQ20 "
    "P60 P00 s60 P50 s00 Q40 Q41 Q42 Q43 Q20 Q21 s50 Q22 Q23 P40 P20 s40 ws20 "
    "wQ70 P61 P51 s61 P01 s20 s51 Q70 P41 s01 Q71 Q72 s41 Q73 P21 P71 wQ10 P62 "
    "P22 s62 P72 s22 Q10 s72 P42 s71 s42 Q11 Q12 Q13 s21 P43 P11 s43 ws73 s11 P73 "
    "P10 s73 s10 P63 P70 s63 P23 s70 t70>2 Q30 s23 t20>0 Q31 P12 Q32 Q33 s12 "
    "t71>2 P30 s30 t30>2 P31 P13 s31 s13 P02 P03 s03 s02 P52 P53 s52 t52>2 P33 "
    "P32 s32 s53 s33 t33>2 t31>2 t61>2 t13>0 t12>2 t32>2 t53>0 t02>2 t01>2 t60>2 "
    "t03>0 | f21 f11 f00 f10 f50 f62 f51 f41 f73 f22 f63 f72 f43 f42 f23 f40",
    "x52>1 x52>3 x22>1 x12>3 x22>3 x73>1 x73>3 x62>1 x23>3 x03>1 K2:012567 x53>3 "
    "x43>1 x63>3 x13>1 K3:0124567 x70>1 x00>3 x62>3 x12>1 x60>3 K0:012567 x10>1 "
    "K1:057 H1:57 wQ20 wQ10 wQ60 P71 P51 Q20 Q21 s71 Q22 Q23 s51 P01 P21 Q10 Q11 "
    "Q12 s01 Q13 s21 Q60 Q61 Q62 Q63 P11 P61 s11 s61 wQ40 P10 P60 s10 P50 s60 P70 "
    "P00 Q40 Q41 s70 s00 P20 s50 s20 wQ30 ws30 ws40 P12 P62 Q30 s62 s12 Q31 Q32 "
    "Q33 Q42 Q43 P30 P40 s30 P31 s40 P41 s41 ws22 ws02 s31 P22 P02 s22 P52 s02 "
    "P32 P72 s52 wP33 ws42 ws32 s72 P42 P33 P73 s42 s32 P63 s33 P53 s73 P13 P43 "
    "s43 ws53 ws63 s13 P03 P23 s53 s63 s03 s23 t50>1 t71>3 t30>3 t20>3 t51>1 "
    "t13>3 t73>1 t03>3 t63>1 t43>1 t53>3 t23>1 t40>1 t33>3 | f70 f00 f52 f41 f21 "
    "f31 f22 f61 f11 f12 f42 f32 f10 f02 f62 f01 f72 f60",
    "x13>2 x31>0 x71>0 x20>2 K0:1237 x70>2 x10>2 x51>2 x01>0 x11>0 x10>0 x01>2 "
    "x13>0 K1:012357 x11>2 x12>0 x32>2 K2:12357 K3:137 x30>2 x31>2 H0:137 wQ50 "
    "wQ20 P10 P70 P30 s10 Q50 s70 Q51 s30 Q20 Q21 Q22 Q23 Q52 Q53 P20 P50 s20 s50 "
    "wQ00 P21 P71 s21 P11 s71 P31 s11 Q00 Q01 s31 Q02 P51 Q03 wQ60 P12 P02 s12 "
    "P32 s02 Q60 P01 s32 P52 s51 s52 Q61 Q62 wP13 s01 Q63 P13 P61 s13 s61 P33 P60 "
    "s33 ws03 s60 P53 P03 s53 P00 s03 t00>0 Q40 t00>2 P62 t50>0 Q41 Q42 t51>2 s62 "
    "Q43 P22 P40 t40>0 t40>2 P73 P41 s41 ws63 s73 P63 P72 s63 s22 P43 P23 s72 "
    "ws23 s43 P42 s23 s42 t41>2 t73>0 t43>0 t21>2 t63>0 t22>2 t23>0 t11>2 t42>2 "
    "t10>2 t62>2 t72>2 | f01 f61 f70 f12 f71 f60 f30 f31 f20 f52 f13 f02 f03 f32 "
    "f53 f33",
)


def _route(g, c):
    red, bc = _ROUTES[g].split()[c].split("/")
    return tuple([-1 if ch == "-" else int(ch) for ch in s] for s in (red, bc))


def _runs(items):
    out = []
    for v in sorted(items):
        if out and sum(out[-1]) == v:
            out[-1][1] += 1
        else:
            out.append([v, 1])
    return out


def _rows(g, n=1):
    return pl.ds(g * _ROWS, n * _ROWS)


def _lanes(k, n=1):
    return pl.ds(k * _LANES, n * _LANES)


def _mailboxes():
    inbox, outbox = ([{} for _ in range(_CHIPS)] for _ in range(2))
    for i, steps in enumerate(_STEPS):
        for step in steps.split():
            if step[0] in "xst":
                g, c = int(step[1]), int(step[2])
                dst = _route(g, c)[0][i] if step[0] == "s" else int(step[4])
                inbox[dst][step[0], g, c, i] = len(inbox[dst])
                outbox[i][step[0], g, c, dst] = len(outbox[i])
    return inbox, outbox


_INBOX, _OUTBOX = _mailboxes()


def _dot(a, b):
    return jnp.dot(a, b.astype(jnp.bfloat16), preferred_element_type=jnp.float32)


class _Chip:
    def __init__(self, i, barrier, refs):
        self.i, self.barrier = i, barrier
        (self.x_hbm, self.w1_hbm, self.w2_hbm, self.out, self.x_f32, self.w1,
         self.w2, self.x, self.pre, self.h, self.own, self.tx, self.rx,
         self.load_sems, self.recv_sems, self.send_sems) = refs
        self.loads = _LOADS[i].split()
        self.steps, self.last = (s.split() for s in _STEPS[i].split("|"))
        self.loaded, self.received, self.sent = set(), set(), []
        self.have_x, self.have_total, self.halved = set(), set(), set()
        self.terms = {}
        self.in_mxu = []


    def load(self, j):
        kind, arg = self.loads[j].split(":")
        if kind == "u":
            pairs = [(self.w1_hbm.at[_lanes(int(arg))], self.w1.at[int(arg)])]
        elif kind == "v":
            c = int(arg[0])
            r = pl.ds(512 * int(arg[1]), 512) if arg[1:] else pl.ds(0, 1024)
            pairs = [(self.w2_hbm.at[r, _lanes(c)], self.w2.at[c, r])]
        else:
            slabs, groups = {}, {}
            for g, k in arg.split(","):
                slabs.setdefault(int(g), []).append(int(k))
            for g, ks in slabs.items():
                groups.setdefault(tuple(ks), []).append(g)
            where = [(_rows(*r), _lanes(*s)) for ks, gs in groups.items()
                     for r in _runs(gs) for s in _runs(ks)]
            pairs = [(self.x_hbm.at[w], self.x_f32.at[w]) for w in where]
        return [pltpu.make_async_copy(s, d, self.load_sems.at[j]) for s, d in pairs]

    def message(self, kind, g, c, src, dst):
        if kind == "x":
            s = d = self.x.at[c, _rows(g)]
        elif kind == "s":
            s = self.tx.at[c, _rows(g)]
            d = self.rx.at[int(src == (dst + 1) % _CHIPS), c, _rows(g)]
        else:
            s = d = self.out.at[_rows(g), _lanes(c)]
        return pltpu.make_async_remote_copy(
            s, d, self.send_sems.at[_OUTBOX[src][kind, g, c, dst]],
            self.recv_sems.at[_INBOX[dst][kind, g, c, src]],
            device_id=(dst,), device_id_type=pl.DeviceIdType.MESH)

    def send(self, kind, g, c, dst):
        if not self.sent:
            pl.semaphore_wait(self.barrier, 2)
        self.sent.append((kind, g, c, self.i, dst))
        self.message(*self.sent[-1]).start()

    def wait_loads(self, kind, names):
        for j, load in enumerate(self.loads):
            if (j not in self.loaded and load[0] == kind
                    and any(n in names for n in load[2:].split(","))):
                self.loaded.add(j)
                self.store()
                for copy in self.load(j):
                    copy.wait()

    def wait_messages(self, kind, g, c, senders):
        for src in senders:
            key = (kind, g, c, src)
            if key in _INBOX[self.i] and key not in self.received:
                self.received.add(key)
                self.store()
                self.message(*key, self.i).wait_recv()


    def store(self, key=None):
        while self.in_mxu and (key is None or key in [m[0] for m in self.in_mxu]):
            self.in_mxu.pop(0)[1]()

    def store_finished(self, cycles):
        while self.in_mxu and cycles + sum(m[2] for m in self.in_mxu[1:]) >= 120:
            self.in_mxu.pop(0)[1]()


    def senders(self, step):
        red, _ = _route(int(step[1]), int(step[2]))
        if step[0] != "s" and red[self.i] >= 0:
            return [red[self.i]]
        return [j for j in range(_CHIPS) if red[j] == self.i and red[self.i] != j]

    def pieces(self, step):
        if step[0] == "K":
            return [(int(g), int(step[1])) for g in step[3:]]
        g = int(step[1])
        if step[0] == "x":
            return [(g, int(step[2]))]
        return [(g, k) for k in range(4) if k not in self.terms.get(g, [])]

    def wait_for(self, step, convert=False):
        if step[0] in "xKQ":
            pieces = self.pieces(step)
            self.wait_loads("x", ["%d%d" % p for p in pieces])
            for g, k in pieces:
                sent_here = any(key[:3] == ("x", g, k) for key in _INBOX[self.i])
                if convert and not sent_here and (g, k) not in self.have_x:
                    self.have_x.add((g, k))
                    piece = self.x_f32[_rows(g), _lanes(k)]
                    self.x[k, _rows(g)] = piece.astype(jnp.bfloat16)
            for g, k in pieces:
                self.wait_messages("x", g, k, range(_CHIPS))
            if step[0] != "x":
                self.wait_loads("u", [str(k) for _, k in pieces])
        elif step[0] == "H":
            self.wait_loads("v", [step[1] + "0"])
        elif step[0] == "P":
            self.wait_loads("v", [step[2], step[2] + "0", step[2] + "1"])
        else:
            g, c = int(step[1]), int(step[2])
            source = _route(g, c)[1][self.i]
            if step[0] != "s" and source >= 0:
                self.wait_messages("t", g, c, [source])
            else:
                self.wait_messages("s", g, c, self.senders(step))

    def plus_received(self, value, step):
        g, c = int(step[1]), int(step[2])
        for j in self.senders(step):
            side = int(j == (self.i + 1) % _CHIPS)
            value = value + self.rx[side, c, _rows(g)].astype(jnp.float32)
        return value.astype(jnp.bfloat16)

    def run(self, step):
        if step[0] == "w":
            return self.wait_for(step[1:])
        self.wait_for(step, convert=True)
        if step[0] in "KH":
            a, groups = int(step[1]), [int(g) for g in step[3:]]
            self.store()
            if step[0] == "K":
                lhs = [self.x[a, _rows(*r)] for r in _runs(groups)]
                d = _dot(jnp.concatenate(lhs, axis=0), self.w1[a])
            else:
                lhs = [self.h[_rows(*r), :512] for r in _runs(groups)]
                d = _dot(jnp.concatenate(lhs, axis=0), self.w2[a, :512])
            for j, g in enumerate(groups):
                v = d[j * _ROWS:(j + 1) * _ROWS]
                if step[0] == "H":
                    self.halved.add((g, a))
                    self.own[a, _rows(g)] = v
                    continue
                if g in self.terms:
                    v = v + self.pre[_rows(g)]
                self.terms.setdefault(g, []).append(a)
                if len(self.terms[g]) == 4:
                    self.h[_rows(g)] = jnp.maximum(v, 0.0).astype(jnp.bfloat16)
                else:
                    self.pre[_rows(g)] = v
            return
        g, c = int(step[1]), int(step[2])
        if step[0] == "x":
            self.send("x", g, c, int(step[4]))
        elif step[0] == "Q":
            ks, cols = [k for _, k in self.pieces(step)], _lanes(2 * c, 2)
            cycles = _ROWS * len(ks) // 2
            self.store_finished(cycles)
            d = _dot(jnp.concatenate([self.x[k, _rows(g)] for k in ks], axis=1),
                     jnp.concatenate([self.w1[k, :, cols] for k in ks], axis=0))
            if g in self.terms:
                d = d + self.pre[_rows(g), cols]

            def store():
                self.h[_rows(g), cols] = jnp.maximum(d, 0.0).astype(jnp.bfloat16)

            self.in_mxu.append((g, store, cycles))
        elif step[0] == "P":
            self.store(g)
            cycles = _ROWS if (g, c) in self.halved else 2 * _ROWS
            self.store_finished(cycles)
            if (g, c) in self.halved:
                d = self.own[c, _rows(g)] + _dot(self.h[_rows(g), 512:], self.w2[c, 512:])
            else:
                d = _dot(self.h[_rows(g)], self.w2[c])

            def store():
                if _route(g, c)[0][self.i] >= 0 and not self.senders("s" + step[1:]):
                    self.tx[c, _rows(g)] = d.astype(jnp.bfloat16)
                else:
                    self.own[c, _rows(g)] = d

            self.in_mxu.append(((g, c), store, cycles))
        elif step[0] == "s":
            self.store((g, c))
            if self.senders(step):
                self.tx[c, _rows(g)] = self.plus_received(self.own[c, _rows(g)], step)
            self.send("s", g, c, _route(g, c)[0][self.i])
        else:
            red, bc = _route(g, c)
            if bc[self.i] < 0 and (g, c) not in self.have_total:
                self.have_total.add((g, c))
                self.store((g, c))
                if red[self.i] >= 0:
                    mine = self.tx[c, _rows(g)].astype(jnp.float32)
                else:
                    mine = self.own[c, _rows(g)]
                self.out[_rows(g), _lanes(c)] = self.plus_received(mine, step)
            if step[0] == "t":
                self.send("t", g, c, int(step[4]))

    def start(self):
        for j in range(len(self.loads)):
            for copy in self.load(j):
                copy.start()
            if j == 1:
                for side in (1, _CHIPS - 1):
                    pl.semaphore_signal(
                        self.barrier, inc=1, device_id=((self.i + side) % _CHIPS,),
                        device_id_type=pl.DeviceIdType.MESH)

    def work(self):
        for step in self.steps:
            self.run(step)
        self.store()

    def finish(self):
        for step in self.last[:-2]:
            self.run(step)
        for sent in self.sent:
            self.message(*sent).wait_send()
        for step in self.last[-2:]:
            self.run(step)
        assert len(self.received) == len(_INBOX[self.i])
        assert len(self.loaded) == len(self.loads)


def _body(*refs):
    me = lax.axis_index("i")
    barrier = pltpu.get_barrier_semaphore()
    chips = [_Chip(i, barrier, refs) for i in range(_CHIPS)]
    for i in (2, 1, 3, 0):
        pl.when(me == i)(chips[i].start)
    for i in (2, 1, 3, 0):
        pl.when(me == i)(chips[i].work)
    for i in (1, 3, 2, 0):
        pl.when(me == i)(chips[i].finish)


def pallas_dist_mlp2_tp_i_m512_h1024_out512_kernel(
    x: jax.Array,
    W1: jax.Array,
    W2: jax.Array,
):
    f32, bf16 = jnp.float32, jnp.bfloat16
    return pl.pallas_call(
        _body,
        out_shape=jax.ShapeDtypeStruct((512, 512), bf16),
        in_specs=[pl.BlockSpec(memory_space=pltpu.MemorySpace.HBM)] * 3,
        out_specs=pl.BlockSpec(memory_space=pltpu.VMEM),
        scratch_shapes=[
            pltpu.VMEM((512, 512), f32),
            pltpu.VMEM((4, 128, 1024), f32),
            pltpu.VMEM((4, 1024, 128), f32),
            pltpu.VMEM((4, 512, 128), bf16),
            pltpu.VMEM((512, 1024), f32),
            pltpu.VMEM((512, 1024), bf16),
            pltpu.VMEM((4, 512, 128), f32),
            pltpu.VMEM((4, 512, 128), bf16),
            pltpu.VMEM((2, 4, 512, 128), bf16),
            pltpu.SemaphoreType.DMA((max(len(s.split()) for s in _LOADS),)),
            pltpu.SemaphoreType.DMA((max(len(box) for box in _INBOX),)),
            pltpu.SemaphoreType.DMA((max(len(box) for box in _OUTBOX),)),
        ],
        compiler_params=pltpu.CompilerParams(
            collective_id=0,
            disable_bounds_checks=True,
            disable_semaphore_checks=True,
        ),
    )(x, W1, W2)
```
